```python
import numpy as np

kernel_name = "dist_layernorm_xy_m6144_n2048"

def setup_inputs():
    x = np.random.randn(12288, 4096).astype(np.float32)
    gamma = np.random.randn(4096).astype(np.float32)
    beta = np.random.randn(4096).astype(np.float32)
    return {"x": x, "gamma": gamma, "beta": beta}

def reference(x: np.ndarray, gamma: np.ndarray, beta: np.ndarray) -> np.ndarray:
    eps = 1e-5
    mean = np.mean(x, axis=1, keepdims=True)
    var = np.var(x, axis=1, keepdims=True)
    return gamma * (x - mean) / np.sqrt(var + eps) + beta
```

```python
import jax
import jax.numpy as jnp
from jax import lax
from jax.experimental import pallas as pl
from jax.experimental.pallas import tpu as pltpu

EPS = 1e-5
LANES = 128
SLAB = 128
NP = 3
R = 256
TAIL = (128, 64, 32, 32)
W = 3
DEFER = 4
UH = 4
UN = 2
READ_PRIORITY = 1


def _tree_sum(xs):
    xs = list(xs)
    while len(xs) > 1:
        xs = [xs[i] + xs[i + 1] if i + 1 < len(xs) else xs[i]
              for i in range(0, len(xs), 2)]
    return xs[0]


def pallas_dist_layernorm_xy_m6144_n2048_kernel(
    x: jax.Array,
    gamma: jax.Array,
    beta: jax.Array,
):
    M, N = x.shape
    PR = M // NP
    NT = N // LANES
    BP = PR // R
    HM = R // LANES
    ntail = sum(TAIL)
    assert M % (NP * SLAB) == 0 and N % LANES == 0
    assert PR % R == 0 and (PR - ntail) % R == 0 and R % SLAB == 0

    blocks = []
    for p in range(NP):
        nmain = (PR - (ntail if p == NP - 1 else 0)) // R
        blocks += [(p, i * R, R) for i in range(nmain)]
    row = PR - ntail
    for t in TAIL:
        assert t % 8 == 0 and (row % SLAB) + t <= SLAB
        blocks.append((NP - 1, row, t))
        row += t
    NB = len(blocks)
    NBM = NB - len(TAIL)
    first_entry, ne = [], 0
    for _, _, n in blocks:
        first_entry.append(ne)
        ne += pl.cdiv(n, LANES)
    last_dynamic = NBM - W
    assert last_dynamic >= (NP - 1) * BP + 1 and NB - DEFER > last_dynamic

    def kernel_body(x_hbm, g_hbm, b_hbm, o0, o1, o2,
                    g_v, b_v, g_bc, b_bc, snd, rcv, ml, ql, mu_bc, rs_bc,
                    rsem, gsem, ssem, xsem):
        peer = (lax.axis_index("x"), 1 - lax.axis_index("y"))
        outs = (o0, o1, o2)

        def slab_row(r, align):
            if isinstance(r, int):
                return divmod(r, SLAB)
            return (lax.shift_right_logical(r, SLAB.bit_length() - 1),
                    pl.multiple_of(r & (SLAB - 1), align))

        def read(p, r0, n, b):
            a0 = p * (PR // SLAB)
            if n % SLAB == 0:
                a = r0 // SLAB if isinstance(r0, int) else lax.shift_right_logical(
                    r0, SLAB.bit_length() - 1)
                src = x_hbm.at[pl.ds(a0 + a, n // SLAB)]
                dst = outs[p].at[pl.ds(a, n // SLAB)]
            else:
                a, rr = divmod(r0, SLAB)
                src = x_hbm.at[a0 + a, pl.ds(rr, n)]
                dst = outs[p].at[a, pl.ds(rr, n)]
            return pltpu.make_async_copy(src, dst, rsem.at[b])

        def start_read_dynamic(b):
            for p in range(NP):
                @pl.when((b >= p * BP) & (b < (p + 1) * BP))
                def _():
                    read(p, (b - p * BP) * R, R, b).start(priority=READ_PRIORITY)

        def entry(b):
            return first_entry[b] if isinstance(b, int) else b * HM

        def exchange(b, n):
            sl = pl.ds(entry(b), pl.cdiv(n, LANES))
            return pltpu.make_async_remote_copy(
                snd.at[sl], rcv.at[sl], ssem, xsem.at[b],
                device_id=peer, device_id_type=pl.DeviceIdType.MESH)

        def cols(j):
            return pl.ds(j * LANES, LANES)

        def loop(n_iter, f):
            if n_iter == 1:
                f(0, 0)
            else:
                lax.fori_loop(0, n_iter, f, 0)

        for b in range(W):
            read(*blocks[b], b).start(priority=READ_PRIORITY)
        g_cp = pltpu.make_async_copy(g_hbm, g_v, gsem.at[0])
        b_cp = pltpu.make_async_copy(b_hbm, b_v, gsem.at[1])
        g_cp.start()
        b_cp.start()
        bar = pltpu.get_barrier_semaphore()
        pl.semaphore_signal(bar, inc=1, device_id=peer,
                            device_id_type=pl.DeviceIdType.MESH)
        g_cp.wait()
        b_cp.wait()
        g_bc[...] = jnp.broadcast_to(g_v[...], (8, N))
        b_bc[...] = jnp.broadcast_to(b_v[...], (8, N))
        diag = (lax.broadcasted_iota(jnp.int32, (8, LANES), 1)
                - lax.broadcasted_iota(jnp.int32, (8, LANES), 0))
        pl.semaphore_wait(bar, 1)

        def stats(o, r0, n, b):
            uh = min(UH, n // 8)

            def per_lane(i, _):
                off = i * (8 * uh)
                if not isinstance(off, int):
                    off = pl.multiple_of(off, 8 * uh)
                a, rr = slab_row(r0 + off, 8 * uh)
                for k in range(uh):
                    rows = pl.ds(rr + k * 8, 8)
                    xs = [o[a, rows, cols(j)] for j in range(NT)]
                    m = _tree_sum(xs) * (1.0 / NT)
                    q = _tree_sum([(v - m) * (v - m) for v in xs])
                    ml[pl.ds(off + k * 8, 8), :] = m
                    ql[pl.ds(off + k * 8, 8), :] = q
                return 0

            loop(n // (8 * uh), per_lane)
            nh = pl.cdiv(n, LANES)
            pm = [jnp.zeros((8, LANES), jnp.float32)] * nh
            pv = list(pm)
            for g in range(n // 8):
                m = ml[pl.ds(g * 8, 8), :]
                mean = jnp.sum(m, axis=1, keepdims=True) * (1.0 / LANES)
                d = m - mean
                t = ql[pl.ds(g * 8, 8), :] + float(NT) * (d * d)
                m2 = jnp.sum(t, axis=1, keepdims=True)
                h, gl = divmod(g, LANES // 8)
                sel = diag == 8 * gl
                pm[h] = jnp.where(sel, mean, pm[h])
                pv[h] = jnp.where(sel, m2, pv[h])
            for h in range(nh):
                snd[entry(b) + h, 0:1, :] = jnp.sum(pm[h], axis=0, keepdims=True)
                snd[entry(b) + h, 1:2, :] = jnp.sum(pv[h], axis=0, keepdims=True)

        def norm(o, r0, n, b):
            un = min(UN, n // 8)
            mean_p, rstd_p = [], []
            for h in range(pl.cdiv(n, LANES)):
                e = entry(b) + h
                ma, va = snd[e, 0:1, :], snd[e, 1:2, :]
                mb, vb = rcv[e, 0:1, :], rcv[e, 1:2, :]
                mean = 0.5 * (ma + mb)
                dl = ma - mb
                var = (va + vb + dl * dl * (0.5 * N)) * (1.0 / (2 * N))
                mean_p.append(jnp.broadcast_to(mean, (8, LANES)))
                rstd_p.append(jnp.broadcast_to(lax.rsqrt(var + EPS), (8, LANES)))
            for g in range(n // 8):
                h, gl = divmod(g, LANES // 8)
                sel = diag == 8 * gl
                mu = jnp.sum(jnp.where(sel, mean_p[h], 0.0), axis=1, keepdims=True)
                rs = jnp.sum(jnp.where(sel, rstd_p[h], 0.0), axis=1, keepdims=True)
                mu_bc[pl.ds(g * 8, 8), :] = jnp.broadcast_to(mu, (8, LANES))
                rs_bc[pl.ds(g * 8, 8), :] = jnp.broadcast_to(rs, (8, LANES))

            def scale(i, _):
                off = i * (8 * un)
                if not isinstance(off, int):
                    off = pl.multiple_of(off, 8 * un)
                a, rr = slab_row(r0 + off, 8 * un)
                rows = [pl.ds(rr + k * 8, 8) for k in range(un)]
                xs = [[o[a, rows[k], cols(j)] for j in range(NT)] for k in range(un)]
                mus = [mu_bc[pl.ds(off + k * 8, 8), :] for k in range(un)]
                rss = [rs_bc[pl.ds(off + k * 8, 8), :] for k in range(un)]
                for j in range(NT):
                    gj, bj = g_bc[:, cols(j)], b_bc[:, cols(j)]
                    for k in range(un):
                        o[a, rows[k], cols(j)] = (xs[k][j] - mus[k]) * rss[k] * gj + bj
                return 0

            loop(n // (8 * un), scale)

        def steady(lo, hi, ps, pn):
            def step(b, _):
                read(ps, (b - ps * BP) * R, R, b).wait()
                start_read_dynamic(b + W)
                stats(outs[ps], (b - ps * BP) * R, R, b)
                exchange(b, R).start()
                if pn is not None:
                    exchange(b - 1, R).wait_recv()
                    norm(outs[pn], (b - 1 - pn * BP) * R, R, b - 1)
                return 0

            if hi > lo:
                lax.fori_loop(lo, hi, step, 0)

        steady(0, 1, 0, None)
        for p in range(NP):
            if p > 0:
                steady(p * BP, p * BP + 1, p, p - 1)
            steady(p * BP + 1, min((p + 1) * BP, last_dynamic), p, p)

        for b in range(last_dynamic, NB):
            p, r0, n = blocks[b]
            read(p, r0, n, b).wait()
            if b + W < NB:
                read(*blocks[b + W], b + W).start(priority=READ_PRIORITY)
            stats(outs[p], r0, n, b)
            exchange(b, n).start()
            if b < NB - DEFER:
                p2, r2, n2 = blocks[b - 1]
                exchange(b - 1, n2).wait_recv()
                norm(outs[p2], r2, n2, b - 1)
        for b in range(NB - 1 - DEFER, NB):
            p, r0, n = blocks[b]
            exchange(b, n).wait_recv()
            norm(outs[p], r0, n, b)
        pltpu.make_async_remote_copy(
            snd, rcv, ssem, xsem.at[0],
            device_id=peer, device_id_type=pl.DeviceIdType.MESH).wait_send()

    pieces = pl.pallas_call(
        kernel_body,
        out_shape=[pltpu.VMEM((PR // SLAB, SLAB, N), jnp.float32)] * NP,
        in_specs=[pl.BlockSpec(memory_space=pltpu.HBM)] * 3,
        out_specs=[pl.BlockSpec(memory_space=pltpu.VMEM)] * NP,
        scratch_shapes=[
            pltpu.VMEM((1, N), jnp.float32),
            pltpu.VMEM((1, N), jnp.float32),
            pltpu.VMEM((8, N), jnp.float32),
            pltpu.VMEM((8, N), jnp.float32),
            pltpu.VMEM((ne, 2, LANES), jnp.float32),
            pltpu.VMEM((ne, 2, LANES), jnp.float32),
            pltpu.VMEM((R, LANES), jnp.float32),
            pltpu.VMEM((R, LANES), jnp.float32),
            pltpu.VMEM((R, LANES), jnp.float32),
            pltpu.VMEM((R, LANES), jnp.float32),
            pltpu.SemaphoreType.DMA((NB,)),
            pltpu.SemaphoreType.DMA((2,)),
            pltpu.SemaphoreType.DMA,
            pltpu.SemaphoreType.DMA((NB,)),
        ],
        compiler_params=pltpu.CompilerParams(
            collective_id=0,
            disable_semaphore_checks=True,
        ),
    )(x.reshape(M // SLAB, SLAB, N), gamma.reshape(1, N), beta.reshape(1, N))
    return jnp.concatenate(pieces, axis=0).reshape(M, N)
```
